```python
import numpy as np

kernel_name = "dist_mlp2_tp_i_m512_h1024_out512"

def setup_inputs():
    x = np.random.randn(512, 512).astype(np.float32)
    W1 = np.random.randn(512, 4096).astype(np.float32)
    W2 = np.random.randn(4096, 512).astype(np.float32)
    return {"x": x, "W1": W1, "W2": W2}

def reference(x: np.ndarray, W1: np.ndarray, W2: np.ndarray) -> np.ndarray:
    h = x @ W1
    h = np.maximum(h, 0.0)
    return h @ W2
```

```python
import contextlib
import jax
import jax.numpy as jnp
from jax import lax
from jax.experimental import pallas as pl
from jax.experimental.pallas import tpu as pltpu

MESH = pl.DeviceIdType.MESH
BF = jnp.bfloat16
F32 = jnp.float32


def make(scopes=False):
    scope = jax.named_scope if scopes else (lambda n: contextlib.nullcontext())

    def body(x_hbm, w1_hbm, w2_hbm, out, xv, w1v, w2v, xb, hb, s1s, s1r, s2s, s2r, lsem, ssem, rsem):
        my = lax.axis_index("i")
        pa = my ^ 1
        pb = 3 - my
        ca = ((my + 1) >> 1) & 1
        cb = my >> 1
        rows = [(1 - ca) * 128, 256 + (1 - cb) * 128, ca * 128, 256 + cb * 128]
        rows = [pl.multiple_of(r, 128) for r in rows]
        loads = {}
        def ld(name, src, dst):
            cp = pltpu.make_async_copy(src, dst, lsem.at[len(loads)])
            cp.start()
            loads[name] = cp
        for g in range(4):
            ld(("x", g), x_hbm.at[pl.ds(rows[g], 128)], xv.at[pl.ds(128 * g, 128)])
        for j in range(2):
            ld(("w1", j), w1_hbm.at[:, pl.ds(512 * j, 512)], w1v.at[j])
        for c in range(4):
            ld(("w2", c), w2_hbm.at[:, pl.ds(128 * c, 128)], w2v.at[c])
        bar = pltpu.get_barrier_semaphore()
        for n in (pa, pb):
            pl.semaphore_signal(bar, inc=1, device_id=(n,), device_id_type=MESH)
        with scope("x"):
            for g in range(4):
                loads["x", g].wait()
                xb[pl.ds(128 * g, 128), :] = xv[pl.ds(128 * g, 128), :].astype(BF)
        for j in range(2):
            with scope(f"w1wait{j}"):
                loads["w1", j].wait()
            with scope(f"h{j}"):
                h = jnp.dot(xb[...], w1v[j].astype(BF), preferred_element_type=F32)
                hb[:, pl.ds(512 * j, 512)] = jnp.maximum(h, 0.0).astype(BF)
        with scope("bar"):
            pl.semaphore_wait(bar, 2)
        part = (pa, pb)
        def rc(step, c, k, src, dst, dev):
            i = (step * 4 + c) * 2 + k
            return pltpu.make_async_remote_copy(src, dst, ssem.at[i], rsem.at[i], device_id=(dev,), device_id_type=MESH)
        d1 = {}; d2 = {}; d3 = {}
        def step1(c):
            with scope(f"w2wait{c}"):
                loads["w2", c].wait()
            with scope(f"s1_{c}"):
                p = jnp.dot(hb[pl.ds(0, 256), :], w2v[c].astype(BF), preferred_element_type=F32)
                s1s[c] = p.astype(BF)
                for k in range(2):
                    d1[c, k] = rc(0, c, k, s1s.at[c, pl.ds(128 * k, 128)], s1r.at[c, pl.ds(128 * k, 128)], part[k])
                    d1[c, k].start()
        def step2(c):
            with scope(f"s2mm_{c}"):
                p = jnp.dot(hb[pl.ds(256, 256), :], w2v[c].astype(BF), preferred_element_type=F32)
            with scope(f"s2wait_{c}"):
                for k in range(2):
                    d1[c, k].wait_recv()
            with scope(f"s2_{c}"):
                s2s[c] = (p + s1r[c].astype(F32)).astype(BF)
                for k in range(2):
                    d2[c, k] = rc(1, c, k, s2s.at[c, pl.ds(128 * k, 128)], s2r.at[c, pl.ds(128 * k, 128)], part[1 - k])
                    d2[c, k].start()
        def step3(c):
            with scope(f"s3wait_{c}"):
                for k in range(2):
                    d2[c, k].wait_recv()
            with scope(f"s3_{c}"):
                f = (s2s[c].astype(F32) + s2r[c].astype(F32)).astype(BF)
                for k in range(2):
                    dst = out.at[pl.ds(rows[2 + k], 128), pl.ds(128 * c, 128)]
                    out[pl.ds(rows[2 + k], 128), pl.ds(128 * c, 128)] = f[128 * k:128 * (k + 1)]
                    d3[c, k] = rc(2, c, k, dst, dst, part[k])
                    d3[c, k].start()
        step1(0); step1(1); step1(2); step2(0); step1(3); step2(1); step2(2); step2(3)
        for c in range(4):
            step3(c)
        with scope("fin"):
            for c in range(4):
                for k in range(2):
                    d1[c, k].wait_send(); d2[c, k].wait_send(); d3[c, k].wait_send()
                    d3[c, k].wait_recv()

    def fn(x, W1, W2):
        ANY = pl.BlockSpec(memory_space=pl.ANY)
        return pl.pallas_call(
            body,
            out_shape=jax.ShapeDtypeStruct((512, 512), BF),
            in_specs=[ANY] * 3,
            out_specs=pl.BlockSpec(memory_space=pltpu.VMEM),
            scratch_shapes=[
                pltpu.VMEM((512, 512), F32), pltpu.VMEM((2, 512, 512), F32), pltpu.VMEM((4, 1024, 128), F32),
                pltpu.VMEM((512, 512), BF), pltpu.VMEM((512, 1024), BF),
                pltpu.VMEM((4, 256, 128), BF), pltpu.VMEM((4, 256, 128), BF),
                pltpu.VMEM((4, 256, 128), BF), pltpu.VMEM((4, 256, 128), BF),
                pltpu.SemaphoreType.DMA((10,)), pltpu.SemaphoreType.DMA((24,)), pltpu.SemaphoreType.DMA((24,)),
            ],
            compiler_params=pltpu.CompilerParams(collective_id=0, disable_semaphore_checks=True, disable_bounds_checks=True),
        )(x, W1, W2)
    return fn


def pallas_dist_mlp2_tp_i_m512_h1024_out512_kernel(x, W1, W2):
    return make()(x, W1, W2)
```

```python
import jax
import jax.numpy as jnp
from jax import lax
from jax.experimental import pallas as pl
from jax.experimental.pallas import tpu as pltpu

_CHIPS = 4
_GROUPS = 16
_ROWS = 32
_LANES = 128
_COMBS, _COMB_ROWS = 4, 8

_ROUTES = {
    "P": "30 21 01 10 03! 12!",
    "P0": "30 21 10 01! 03! 12!",
    "Pb": "30 21 01 10 03! 32!",
    "Q2": "01 32 12 21! 10! 23!",
    "Qr": "01 32 21 10! 12! 23!",
    "Qx": "01 32 12 21 10! 23!",
    "Ua": "32 21 01 10 12! 03!",
    "Ur": "01 32 21 10! 12! 03!",
    "Ux": "01 32 12 21 10! 03!",
}

_TILE_ROUTES = (
    "P' P Pb Qr",
    "P P' Pb' Qr'",
    "P Pb Pb Ua",
    "P' Pb' Pb' Ua'",
    "P Pb' Ua Ua",
    "P' Pb Ua' Ua'",
    "P0 P P0 Ua",
    "P0' P' P0' Ua'",
    "Qr Qr Ur Q2",
    "Qr' Qr' Ur' Q2'",
    "Qr Qr Qr Ur",
    "Qr' Qr' Qr' Ur'",
    "Ux Qr Qx Qr",
    "Ux' Qr' Qx' Qr'",
    "Qr Qx Ur Qx",
    "Qr' Qx' Ur' Qx'",
)

_ROW_SLOT = (
    (12, 13, 10, 11, 7, 2, 15, 14, 0, 1, 4, 3, 6, 5, 9, 8),
    (0, 1, 2, 3, 4, 5, 6, 7, 8, 9, 10, 11, 12, 13, 14, 15),
    (0, 1, 2, 3, 4, 5, 6, 7, 8, 9, 10, 11, 12, 13, 14, 15),
    (1, 0, 3, 2, 5, 4, 7, 6, 9, 8, 11, 10, 13, 12, 15, 14),
)
_COL_SLOT = ((2, 3, 0, 1), (0, 1, 2, 3), (0, 1, 2, 3), (0, 1, 2, 3))

_PROGRAM_OF_CHIP = ("even", "odd", "even", "odd")
_MATMULS = {
    "odd": (
        "h00:b",
        "h00:3f",
        "h00:17",
        "h0*:0d h01:3",
        "h01:17bf",
        "h0*:45 h10:013457bdf",
        "h0*:9 h1*:9 h11:013457bdf",
        "o00:4 o0*:3579bd",
        "o00:1 o0*:0f o11:179bdf",
        "o10:179bdf o1*:34",
        "h0*:2 h1*:2 o01:4 o21:179bf",
        "o20:19b o2*:3",
        "h0*:6 h1*:6 o20:7f o2*:5",
        "o0*:26 o01:1 o3*:1b",
        "o10:6 o1*:2 o11:0 o3*:357",
        "o1*:5 o11:6 o2*:d o21:6 o3*:df",
        "h0*:8 h1*:8 o10:0",
        "o0*:8 o20:6",
        "o1*:8 o2*:28 o3*:8",
        "h0*:a h1*:a o2*:0",
        "o0*:a o1*:a o20:4 o21:a o3*:9",
        "h1*:c o20:a o21:4 o30:0 o31:a",
        "h0*:c h10:e o30:6a o31:0",
        "h11:e o1*:c o2*:c o3*:4 o31:c",
        "h0*:e o30:c o31:6",
        "o0*:ce o3*:e",
        "o1*:e o21:e o3*:2",
        "o20:e",
    ),
    "even": (
        "h01:28",
        "h01:9",
        "h00:289 h0*:01345",
        "h0*:67 h10:0123456789",
        "h00:b h1*:b h11:0123456789",
        "o0*:0145",
        "o0*:23678 o01:9",
        "o00:9 o1*:2346",
        "o10:8 o1*:01579",
        "o11:8 o2*:012367",
        "h0*:a h01:b h1*:a o20:4 o0*:ab o1*:ab o2*:89a",
        "o2*:5b o21:4 o3*:01 o31:a",
        "h0*:cd h1*:cd o30:a o3*:b",
        "o1*:cd o3*:4567",
        "o0*:cd o2*:cd o3*:23cd",
        "h0*:ef h1*:ef o0*:ef o2*:ef",
        "o1*:ef o3*:ef",
        "o3*:89",
    ),
}

_STEPS = (
    (
        "Gxe Gxa Gx4 Gxd E Gx9 Gxc Gx5 Gxf Gxb Ga01 Lxd Lxc Lxe Lx5 C5 Cd Lx4 Cc Gx8 Lxf Lx9 "
        "Ga00 Cf Ga10 Lxa Lxb C4 Ga11 Ce Cb C9 Gb20 B xc>3 xd>1 Lx8 x5>1 x4>3 xc>1 La01 C8 Ca "
        "Gb21",
        "xf>3 xd>3 xe>1",
        "Gb30 Gb31 La00",
        "Gb00 La10",
        "La11 Gb01 x3<1",
        "Lb20 Lb21",
        "p82>1 p92>3 pd2>3",
        "p42>1 Lb30 Gb10 Gb11 Lb31 pf2>3 pa2>1 pb2>3 pc2>1",
        "pa3>1 p52>3",
        "p43>1 pc3>1 pd3>3 pe2>1 pe3>1 Lb00 Lb01 p53>3 pb3>3",
        "x2<3 pf3>3 Lb10 p80>1 p90>3 pc0>1 x0<1 pb0>3",
        "p33>3 Lb11 pe0>1 p93>3 p23>1 x1<3 pa2!1 p83>1",
        "pf0>3 p50<1 p40<3 pa0>1 p81>1 p20<3 p30<1 A20 A50 A30 A40 p20>1 p50>3 p91>3 p30>3 "
        "p40>1",
        "pd0>3",
        "p92!3 pd1>3 pc1>1 p31<1 pa1>1 xe!1 p41<1 p10<3 A31 p61<3 p01<3 p50!3 pf3!3 p03>1 "
        "p31>3 p13>3",
        "pb1>3 x6<3 p70<1 p21<3 x7<1 A41 A01 p01>1 p60<3 p41>3 p51<3 pf2!3 A10 p71<1 A21 "
        "p11<1 p02<3 p10>1 A11 p00<1 pa3!1 A02 p02>1 pe3!1 p22<3 p12<1 A00 p32<1 p21>1 p93!3 "
        "p62<3 A22 p22>1 A12 p12>3 pc0!1 p00>3 A51 p11>3",
        "p40<1 p50<3 p60<1 p01!1 p00<3 p31<3 xd!1 p51>1 p90!3 p21<1 F00 p70<3 A32 p10<1 p32>3 "
        "f00>1 F40 p53!3 f40>3 F31 F21 p52!3",
        "p30<3 A71 pa1!1 p71>3 A61 p02!1 p61>1 F30 f21>3 f31>1 p51<1 pb3!3 p61<1 F10 F60 F70",
        "f10>3 p83!1 p41<3 p11<3 p63>1 p20<1 p01<1 p40!1 p71<3 p62<1 F20 p72<1 f00!1 p33!3 "
        "F41 pa0!1 f70>3 xc!1 f60>1 F62 F01 f01>3 f62>1 p72<3 xd!3 pf1>3 xf!3 f81<1 F72 pe1>1 "
        "f60>3 f72>3 F61 f72>1 F50 p02<1 f60!1 p12<3 p73>3 x4!3 f50>1 pe0!1 xc!3 p10!1 F51 "
        "pe1!1 p22<1 f20>3 pb0!3 f70>1 f41>1 f92<3 f30>1 p42<1 p23!1 f51>3 p00!3 f92>1 f61>3 "
        "F02 pc2!1 f02>3 F71 f20!3 F22 p52<3 fa3<1 fb0<3 f10!3 f62>3 f71>1 F42 p32<3 F11 "
        "f11>1 fa1<1 F12 fa3>3 F52 pb1!3 p61!1 f60!3 fb3<3 f52>1 fb3>1 p43<1 p41!3 f22>3 F32 "
        "p32!3 p53<3 p11!3 f42>3 f02!3 f32>1 F53 p63<1 fb2<3 f53>1 p80!1 f82<1 f12>1 F43 "
        "f61!3 pc3!1 p42!1 fc1<1 f11!1 f82>3 p73<3 fd1<3 f43>3 p82!1 fc2<1 F73 p31!3 pe2!1 "
        "f73>1 f32!1 F63 f70!3 p03!1 f80<1 f92!1 fc0<1 f63>3 pc1!1 p51!1 f70!1 pb2!3 f82!3 "
        "fc0>3 fa3!3 fd0<3 f52!1 p23<1 fd0>1 f72!3 pf1!3 p22!1 pf0!3 F23 p43!1 f90<3 p20!1 "
        "f41!1 fa2<1 p33<3 f71!1 F33 f33>1 f21!3 f23>3 fe2<1 fe2>3 p81!1 ff2<3 ff2>1 f62!3 "
        "p91!3 fe3<1 x5!1 pd3!3 f01!3 fe1<1 fc3<1 fe0<1 f23!3 f03<1 f42!3 f22!3 f73!1 f51!3 "
        "ff1<3 p71!3 f31!1 fa0<1 ff0<3 p73!3 fc0!3 f12!1 pd0!3 f30!1 f43!3 f40!3 f62!1 fd0!1 "
        "f63!3 p30!3 ff2!1 f72!1 fd2<3 p21!1 fe2!3 f33!1 f91<3 fb3!1 ff3<3 p63!1 fd3<3 f13<3 "
        "fb1<3 p13!3 f53!1 f50!1 pd2!3 p12!3 pd1!3 f83<1 f93<3",
    ),
    (
        "Gx0 E Gx3 Gx7 Gx1 Gxf Gxb Ga00 Lxb Ga01 Lx1 Lx3 Lx7 C3 C1 Lx0 B x3>0 x1>2 Lxf C7 "
        "x7>2 La00 x7>0 Cf Cb Ga10 Ga11 Gb01",
        "xb>2 C0",
        "",
        "xd<0 Gb00 Gb11 xd>2 Gb10 La01",
        "xf>2 Gb21",
        "x0>0 x4<2 La10 x5<0",
        "x9<2 La11",
        "Lb01 Gb20 x2<2 Gb30 Lb00",
        "pd0>2 p50>0 Lb11 p30>0 p90>2 Gb31 p70>0 pb0>2",
        "Lb10 p00>0 pf0>2",
        "p71>0 p11>0 p31>0 p91>2 Lb21 pb1>2 pf1>2 pd1>2",
        "Lb20 p41>0",
        "p12>0 p92>2 pb2>2 x6<2 p32>0",
        "Gxa p40<2 p52>2 pf2>2 p72>0 Lb30 A40 p40>0 Lb31",
        "p10<2 p13>2 pb3>2 p60<2 A10 A60 p10>0 p60>0",
        "p20<2 p21<2 p53>2 A20 A21 p73>2 p21>0 p20>0",
        "p61<2 p51<2 A51 A61 p51>0 pd2>2 pf3>2 p61>0 pd3>2 x8<2",
        "p01<2 A01 p01>0",
        "p62<2 A62 p62>0 p33>2 p83<0 p80<2 p82<0 p80<0 F80 f80>2 f80>0 p81<0",
        "Lxa p22<2 Ca A83 A22 p22>0 p81<2 p83>2 F81 f81>0 f81>2",
        "p82<2 F82 f82>0 f82>2 p02<2 xc<0 p20<0 p40<0 F40 A02 p02>0 f40>2 pa1<0",
        "pa0<2 pa0<0 pf1!2 Fa0 fa0>0 p93>2 F20 pa1<2 pa3<0 Fa1 pd1!2 fa1>0 fa1>2",
        "fa0>2 pc1<0 pa2<0 p42<2 A42 p42>0 p22!0 pe3<0 pa2<2 Fa2 f20>2 xe<0 fa2>0 f82!0",
        "f80!2 fa2>2 p33!2 x3!0 pa3<2 p03<0 Fa3 fa3>0 fa3>2 pc2<0 p22<0 p03<2 F03 f03>0",
        "pc1<2 Fc1 fc1>0 x1!2 fc1>2 pc3<0 p10<0 x7!2 f03>2 Ac2 p43<2 pc0<0 A43 p43>0",
        "pc2>2 p63<2 A63 f31<0 p63>0 xb!2 p61<0 p23<0 p00!0 F10 p51<0 p31!0 p43<0 f10>2 p91!2 "
        "pc3<2 Fc3 fc3>0 fc3>2 fa0!0",
        "pc2<2 Fc2 fc2>0 p50!0 p40!0 pe2<0 Ac0 Ae3 f31>2 p63<0 p83!2 pe0<0 pc0<2 Fc0 fc0>0 "
        "F43",
        "fa2!2 p02!0 p70!0 p23<2 pe1<0 pe3>2 A23 Ae1 p23>0 f60<0 p42<0",
        "xf!2 pe0<2 pe1>2 pd2!2 Fe0 F23 fa1!2 fe0>0 pe2<2 p10!0 fa0!2 fe0>2 Fe2 f40!2 fe2>0 "
        "f20!2 pe1<2 p72!0 p43!0 fe2>2 p90!2 f60>2 Fe1 pc0>2 p01<0 fe1>0 pe3<2 xd!2 Fe3 p93!2 "
        "F01 F61 fe3>0 F63 f41<0 f01>2 f23>2 pb3!2 p73!2 p52!2 fc1!2 p11!0 fa3!2 F42 p30!0 "
        "x0!0 f42>2 f62<0 f81!0 f63>2 pf3!2 p63!0 f62>2 p71!0 p21<0 pb1!2 F21 p53!2 f83<2 "
        "p32!0 f43>2 p42!0 f03!0 f61>2 fc3!2 f83>0 fb0<2 f72<0 f93<2 x7!0 f32<0 pb0!2 f32>2 "
        "f50<0 fc1!0 f60!2 p62!0 fc0!0 p61!0 fc3!0 p21!0 f13<2 f52<0 pc0!2 fe1!0 f12<0 f91<2 "
        "fb1<2 f10!2 f43!2 f53<0 f03!2 p01!0 F51 fe2!0 fe0!2 pc2!2 fb2<2 f41>2 fc2!0 pe3!2 "
        "f71<0 fa2!0 f61!2 pd3!2 f62!2 fd1<2 f70<0 ff1<2 p41!0 f12>2 p02<0 p13!2 f73<0 fd2<2 "
        "pf0!2 fd3<2 pf2!2 f32!2 f92<0 f11<0 f12!2 f81!2 p23!0 f83!0 fe2!2 ff0<2 F02 p12!0 "
        "F22 ff2<0 p51!0 p20!0 f31!2 fd0<0 f33<0 f30<0 p60!0 fb3<0 f63!2 f01!2 p92!2 pe1!2 "
        "f00<0 f23!2 pd0!2 f90<2 fe0!0 fa1!0 f41!2 f42!2 f80!0 fe3!0 fa3!0 f82!2 ff3<2 pb2!2",
    ),
    (
        "Gx4 E Gx5 Gx8 Gx3 Gx2 Gx9 Ga01 Lx4 B Ga00 Ga10 Lx5 Ga11 C5 C4 Gb01 x5>3 x4>1 Lx8 Lx9 "
        "Lx2 Gb00 C8 Lx3 C9 x9>1 Gb10 x8>3 La01 C2 C3 x2>1",
        "x3>3 Gb11",
        "Gb21 x1<1 x8>1 x9>3 x0<3 La00",
        "x7<1 x6<3 x7>3 x6>1 La10",
        "La11 xb<1",
        "Gb20 Lb00 Lb01",
        "p40>1 p50>3 p00>3 p10>1",
        "p70>3 p60>1 Lb10 p20>1 p30>3 Gb31 Gb30 Lb11",
        "p21>1 p31>3 p41>3 p61>1",
        "p51>1 p71>3 p90<1 A90 xc<3 p01>1 xa<3 p80<3 Lb21 A80 xd<1 pa0<3 p11>3 p80>1 pb0<1 "
        "p90>3 Lb20",
        "p81<3 p91<1 p72>3 p62>1 p22>1 A91 A81 p81>1 p91>3 p32>3 p12>3 p02>1",
        "p82<3 p92<1 A92 Ab0 Aa0 A82 p82>1 Lb31 p92>3 Lb30 pb0>3 pa0>1",
        "pa2<3 p42<3 p52<1 pb1<1 pb2<1 pa1<3 A52 Ab1 Aa2 Aa1 Ab2 A42 pb1>3 p52>3 pa1>1 pb2>3 "
        "p42>1 pa2>1",
        "p13<1 p03<3 pa3<3 pb3<1 A03 Ab3 Aa3 A13 pa3>1 p13>3 pd1<1 pb3>3 xf<1 p03>1 pc1<3",
        "Ac1 Ad1 pd1>3 p73<1 pc1>1 p43<3 pc3<3 p53<1 p63<3 A53 A73 A43 A63 pc0<3 p53>3 p73>3 "
        "p43>1 p63>1",
        "pf0<1 pd3<1 p23<3 Ac3 Ad3 pe0<3 pd3>3 pc3>1 pe2<3 pd2<1 pc2<3 p33<1 pd0<1 Ad0 A33 "
        "Ad2 A23 Ac2 Ac0 pd2>3 pc2>1 pc0>1 xe<3 pd0>3 p33>3 p23>1",
        "Af0 Ae0 pf0>3 pe0>1 pf2<1 pc0!1 pe1<3 pf3<1 Af2 Ae2 pf2>3 pe2>1 pe3<3 x8!1",
        "p72!3 pf1<1 Af1 Ae1 Af3 pb3!3 pf1>3 p22!1 pe1>1 p93<1 x5!3 pf3>3 p61!1 x4!1 p93<3 "
        "Ae3 pe3>1 f91<3 p53!3 p40!1 p83<1 pa2!1 x2!1 p83<3 pd0!3",
        "pa3!1 f81<1 x6!1 F83 fb0<3 f80<1 fa1<1 f83>1 F93 f91>1 fa0<1 p03!1 p13!3 p31!3 fb0>1 "
        "pf0!3 f90<3 f93>3 f81>3 f90>1 f52<3 fa0>3 fb1<3 f13<3 pf1!3 p90!3 fa1>3 f83>3 p92!3 "
        "pf2!3 fb1>1 f80>3 p20!1 pb2!3 p02!1 p82!1 fa2<1 f13>1 fb2<3 p51!1 f03<1 f40<1 p21!1 "
        "x9!3 p10!1 f93>1 f03>3 pc3!1 pc2<1 fb2>1 fa2>3 fb3<3 pb1!3 Fc2 fc3<1 fc1<1 fc3>3 "
        "pf3!3 fd1<3 p42!1 fd3<3 p01!1 f90!1 pd2<3 pe1!1 Fd2 fd2>1 p73!3 fd1>1 x3!3 fb0!1 "
        "fc2>3 p23!1 p12!3 fc1>3 p11!3 pf1<3 Ff1 ff1>1 pe1<1 f03!3 fd3>1 Fe1 fe1>3 pe3<1 "
        "pa1!1 ff0<3 x7!3 ff0>1 Fe3 f92<3 fe3>3 pf3<3 fe0<1 p52!3 f83!1 Ff3 ff3>1 f30<3 f93!1 "
        "p50!3 fa1!3 p81!1 p00!3 fe0>3 f53<3 fc3!3 p63!1 f50<3 pc2!1 f81!3 fd2!1 p62!1 f63<1 "
        "f00<3 pc1!1 p43!1 fe0!3 fd3!1 pb0!3 fe3!3 p91!3 f91!1 p33!3 f70<3 f11<3 f31<1 pd2!3 "
        "f82<1 f13!1 f61<1 x9!1 f43<1 ff3!1 ff1!1 p60!1 f20<1 p32!3 f01<1 f80!3 pe0!1 fe2<1 "
        "f02<3 fb2!1 pd3!3 f51<3 fa0!3 f10<1 f83!3 f71<3 pe2!1 f60<1 fd1!1 f33<3 pd1!3 f93!3 "
        "fa2!3 fc1!3 fa3<1 fb1!1 p71!3 f21<3 pc0<1 f32<1 p70!3 f23<1 pd0<3 f42<1 f72<3 x8!3 "
        "ff2<3 p30!3 p41!3 f62<1 f41<1 Fc0 p80!1 fe1!3 fc2!3 ff0!1 f22<3 Fd0 pa0!1 pe3!1 "
        "f12<1 f73<3",
    ),
    (
        "Gxa E Gx2 Gx6 Gx0 Ga00 Lx2 Gxe Lx6 Gx1 Lx0 Ga01 C0 Ga10 B Lxa Ca Ga11 x0>2 Lx1 C6 "
        "Lxe Gb01 x6>0 x6>2 xa>2 C2 Ce La00 Gb00",
        "Gb11 Gb10 C1",
        "xe>2 x2>0 Gb21",
        "xc<0 La01",
        "x1>0",
        "xc>2 x5<2 x4<0 La10",
        "x8<2 La11",
        "Gb20 Lb01 x3<2 Gb31 Lb00",
        "pa0>2 p20>0 p40>0 p80>2 Lb11",
        "p10>0 pc0>2 pe0>2 p60>0 Gb30 Lb10",
        "Gxb p01>0 p61>0 p81>2 pe1>2 pc1>2 Lb21 p21>0",
        "p51>0 Lb20 x7<2 pa1>2",
        "p82>2 pa2>2 p02>0 p22>0",
        "p62>0 p50<2 Lb31 x9<2 p42>2 Lb30 A50 pe2>2 p50>0",
        "p00<2 pa3>2 p70<2 A70 A00 p03>2 p70>0 p00>0",
        "p31<2 p30<2 A30 A31 p31>0 p30>0 p43>2 p63>2",
        "p41<2 p71<2 A71 A41 p41>0 pc3>2 p23>2 p71>0",
        "pc2>2 p11<2 A11 p90<0 p11>0",
        "p90<2 F90 f90>0 f90>2 pe3>2 p91<0 p92<0 p72<2 p30<0 Lxb A72 F30 p72>0 f30>2",
        "p50<0 p91<2 Cb p32<2 A32 F91 f91>0 f91>2 p32>0",
        "p92<2 F92 p12<2 f92>0 f92>2 p93<0 xd<0 A93 A12 p93>2 p12>0",
        "pb1<0 xf<0 pb3<0 p83>2 p32!0 pb0<2 pe1!2 x2!0 pb0<0 Fb0 fb0>0 p13<0 pd1<0 p33<0 "
        "p52<0 fb0>2 pb2<0 pb1<2 Fb1 pd2<0 fb1>0",
        "p52<2 A52 F52 p52>0 pb2<2 f52>2 fb1>2 F50 Fb2 pd0<0 fb2>0 p42!2 x6!0 f50>2",
        "p13<2 p12<0 F13 f13>0 f13>2 pb3<2 Fb3 fb3>0",
        "pd1<2 Fd1 p93!2 fb2>2 fd1>0 pf3<0 p52!0 pf0<0 p53<2 A53 fd1>2 p53>0 pd3<0 pc1!2 "
        "fb3>2",
        "Ad2 p73<2 A73 pd2>2 f21<0 p73>0 f92!0 pd3<2 fb2!2 Fd3 p53<0 fd3>0",
        "fd3>2 pd2<2 p11<0 Fd2 fd2>0 Af3 F11 pe2!2 x1!0 p32<0 pc0!2 Ad0 pe0!2 pd0<2 Fd0 pf3>2 "
        "fd0>0 p53!0",
        "F53 p33<2 p03!2 A33 pc3!2 pf1<0 f13!2 pa0!2 f90!2 f52!2 p33>0 Af1 pf1>2 xc!2 pf0<2 "
        "p00<0 Ff0 ff0>0 p41!0 ff0>2 f91!0 f21>2 fb0!2 p63!2 F00 pf2<0 p60!0 f70<0",
        "p01!0 p71<0 fd3!0 pf2<2 Ff2 pa1!2 F33 ff2>0 f72<0 p81!2 fb1!0 f11>2 pf1<2 p40!0 Ff1 "
        "ff1>0 fd2!0 x0!2 pd0>2 p73<0 f70>2 pf3<2 p20!0 f00>2 f91!2 p12!0 Ff3 p11!0 ff3>0 "
        "p80!2 pa3!2 ff2>2 f72>2 f01<0 f93<2 f93>0 f33>2 pe3!2 pd0!2 fb0!0 f83<2 f92!2 f40<0 "
        "pd2!2 p72!0 F73 ff0!2 ff0!0 F71 pf1!2 f90!0 p41<0 fd1!2 f62<0 f02<0 f22<0 p73!0 "
        "fd0!0 f51<0 f53>2 fb2!0 f02>2 f22>2 f51>2 fa2<2 F32 f72!2 f10<0 pc2!2 f71>2 f00!2 "
        "fd3!2 p31<0 f60<0 pf3!2 f22!2 p00!0 f73>2 f03<2 p43!2 p61!0 f51!2 f61<0 p23!2 fc1<2 "
        "xe!2 f30!2 p33!0 F31 fa1<2 f02!2 fd1!0 p62!0 ff2!2 f63<0 p50!0 f93!0 p21!0 f71!2 "
        "p71!0 f43<0 pa2!2 fa3<0 f23<0 p51!0 f20<0 p30!0 ff1!0 fb1!2 fe2<0 fb3!0 fa0<2 F12 "
        "fc0<0 p22!0 F41 fe3<2 fe1<2 p83!2 f70!2 f81<2 x6!2 f42<0 p82!2 f50!2 f21!2 p31!0 "
        "f33!2 ff3!0 ff2!0 f53!2 fc2<2 fc3<2 f13!0 f82<0 f80<2 fe0<2 fb3!2 xa!2 p10!0 f73!2 "
        "p70!0 f11!2 p02!0",
    ),
)


def _role(group, col, chip):
    name = _TILE_ROUTES[group].split()[col]
    sends, early, got = False, (), ()
    for msg in _ROUTES[name.rstrip("'")].split():
        src, dst = ((-int(c) if name.endswith("'") else int(c)) % _CHIPS for c in msg[:2])
        if msg.endswith("!"):
            continue
        if src == chip:
            sends, early = True, tuple(c for c in got if c != dst)
        if dst == chip:
            got += (src,)
    return sends, early, tuple(c for c in got if c not in early)


def _number_messages():
    sent, received, sems = [0] * _CHIPS, [0] * _CHIPS, {}
    for src in range(_CHIPS):
        for step in " ".join(_STEPS[src]).split():
            if ">" in step:
                msg, dst = step[:-2], int(step[-1])
                sems[msg, src, dst] = (sent[src], received[dst])
                sent[src] += 1
                received[dst] += 1
    return sems, max(sent), max(received)


def _body(x_hbm, w1_hbm, w2_hbm, out, x_f32, w1, w2, x_bf16, h_acc, h_bf16, p_acc,
          p_send, p_recv, load_sems, send_sems, recv_sems):
    f32, bf16 = jnp.float32, jnp.bfloat16
    me = lax.axis_index("i")
    barrier = pltpu.get_barrier_semaphore()
    sems, _, _ = _number_messages()

    def tile_slot(chip, group, col):
        return _ROW_SLOT[chip][group] * 4 + _COL_SLOT[chip][col]

    def out_tile(group, col):
        return out.at[pl.ds(group * _ROWS, _ROWS), pl.ds(col * _LANES, _LANES)]

    def inbox(chip, src, group, col):
        return p_recv.at[int(src == (chip + 1) % _CHIPS), tile_slot(chip, group, col)]

    def load(chip, name, rows=slice(None)):
        i = int(name[1], 16)
        if name[0] == "x":
            src, dst = x_hbm.at[pl.ds(i * _ROWS, _ROWS)], x_f32.at[_ROW_SLOT[chip][i]]
            sem = i
        elif name[0] == "a":
            k = int(name[2])
            src, dst = w1_hbm.at[pl.ds(256 * k, 256), pl.ds(512 * i, 512)], w1.at[i, k]
            sem = _GROUPS + 2 * i + k
        else:
            k = int(name[2])
            src = w2_hbm.at[pl.ds(16 * k, 16), rows, pl.ds(_LANES * i, _LANES)]
            dst = w2.at[_COL_SLOT[chip][i], k, :, rows]
            sem = _GROUPS + 4 + 2 * i + k
        return pltpu.make_async_copy(src, dst, load_sems.at[sem])

    def remote(msg, src, dst):
        group = int(msg[1], 16)
        if msg[0] == "x":
            src_ref, dst_ref = (x_bf16.at[_ROW_SLOT[c][group]] for c in (src, dst))
        elif msg[0] == "p":
            src_ref = p_send.at[tile_slot(src, group, int(msg[2]))]
            dst_ref = inbox(dst, src, group, int(msg[2]))
        else:
            src_ref = dst_ref = out_tile(group, int(msg[2]))
        send, recv = sems[msg, src, dst]
        return pltpu.make_async_remote_copy(
            src_ref, dst_ref, send_sems.at[send], recv_sems.at[recv],
            device_id=(dst,), device_id_type=pl.DeviceIdType.MESH)

    def communicate(chip, index):
        for step in _STEPS[chip][index].split():
            if step == "E":
                for other in ((chip + 1) % _CHIPS, (chip - 1) % _CHIPS):
                    pl.semaphore_signal(barrier, inc=1, device_id=(other,),
                                        device_id_type=pl.DeviceIdType.MESH)
            elif step == "B":
                pl.semaphore_wait(barrier, 2)
            elif step[:2] == "Gb":
                for comb in range(_COMBS):
                    load(chip, step[1:], pl.ds(comb * _COMB_ROWS, _COMB_ROWS)).start()
            elif step[0] == "G":
                load(chip, step[1:]).start()
            elif step[0] == "L":
                load(chip, step[1:]).wait()
            elif step[0] == "C":
                slot = _ROW_SLOT[chip][int(step[1], 16)]
                for j in range(4):
                    x_bf16[slot, j] = x_f32[slot, :, pl.ds(_LANES * j, _LANES)].astype(bf16)
            elif step[0] in "AF":
                group, col = int(step[1], 16), int(step[2])
                slot = tile_slot(chip, group, col)
                sends, early, late = _role(group, col, chip)
                total = p_send[slot].astype(f32) if step[0] == "F" and sends else p_acc[slot]
                for src in early if step[0] == "A" else late:
                    total = total + inbox(chip, src, group, col)[...].astype(f32)
                dst = p_send.at[slot] if step[0] == "A" else out_tile(group, col)
                dst[...] = total.astype(bf16)
            elif step[-2] == ">":
                remote(step[:-2], chip, int(step[-1])).start()
            elif step[-2] == "<":
                remote(step[:-2], int(step[-1]), chip).wait_recv()
            else:
                remote(step[:-2], chip, int(step[-1])).wait_send()

    def matmuls(burst, chips, half_done):
        fresh = {}
        for item in burst.split():
            kind, j = item[0], int(item[1])
            halves = (0, 1) if item[2] == "*" else (int(item[2]),)
            slots = [int(s, 16) for s in item[4:]]
            if kind == "h":
                prod = None
                for k in halves:
                    for e in range(2):
                        lhs = jnp.concatenate([x_bf16[s, 2 * k + e] for s in slots], axis=0)
                        rhs = w1[j, k, pl.ds(_LANES * e, _LANES), :].astype(bf16)
                        term = jnp.dot(lhs, rhs, preferred_element_type=f32)
                        prod = term if prod is None else prod + term
            else:
                blocks = [4 * k + e for k in halves for e in range(4)]
                lhs = jnp.concatenate([
                    jnp.concatenate([fresh[s, b] if (s, b) in fresh else h_bf16[s, b]
                                     for b in blocks], axis=1) for s in slots], axis=0)
                rhs = jnp.concatenate([w2[j, k].reshape(512, _LANES) for k in halves], axis=0)
                rhs = rhs.astype(bf16)
                prod = jnp.dot(lhs, rhs, preferred_element_type=f32)
            for i, s in enumerate(slots):
                rows = prod[i * _ROWS:(i + 1) * _ROWS]
                resumed = (kind, j, s) in half_done
                complete = resumed or len(halves) == 2
                half_done.append((kind, j, s))
                if kind == "h":
                    for e in range(4):
                        b, v = 4 * j + e, rows[:, _LANES * e:_LANES * (e + 1)]
                        if resumed:
                            v = v + h_acc[s, b]
                        if complete:
                            fresh[s, b] = jnp.maximum(v, 0.0).astype(bf16)
                            h_bf16[s, b] = fresh[s, b]
                        else:
                            h_acc[s, b] = v
                    continue
                if resumed:
                    rows = rows + p_acc[4 * s + j]
                as_is = []
                for chip in chips:
                    sends, early, _ = _role(_ROW_SLOT[chip].index(s), _COL_SLOT[chip].index(j), chip)
                    as_is.append(complete and sends and not early)
                if any(as_is):
                    p_send[4 * s + j] = rows.astype(bf16)
                if not all(as_is):
                    p_acc[4 * s + j] = rows

    def program(name):
        chips = [c for c in range(_CHIPS) if _PROGRAM_OF_CHIP[c] == name]
        half_done = []
        for index in range(len(_MATMULS[name]) + 1):
            for chip in chips:
                if _STEPS[chip][index]:
                    pl.when(me == chip)(lambda: communicate(chip, index))
            if index < len(_MATMULS[name]):
                matmuls(_MATMULS[name][index], chips, half_done)

    pl.when(me % 2 == 1)(lambda: program("odd"))
    pl.when(me % 2 == 0)(lambda: program("even"))


def pallas_dist_mlp2_tp_i_m512_h1024_out512_kernel(
    x: jax.Array,
    W1: jax.Array,
    W2: jax.Array,
):
    f32, bf16 = jnp.float32, jnp.bfloat16
    tiles = 4 * _GROUPS
    _, sends, receives = _number_messages()
    return pl.pallas_call(
        _body,
        out_shape=jax.ShapeDtypeStruct((_GROUPS * _ROWS, 4 * _LANES), bf16),
        in_specs=[pl.BlockSpec(memory_space=pl.ANY)] * 3,
        out_specs=pl.BlockSpec(memory_space=pltpu.VMEM),
        scratch_shapes=[
            pltpu.VMEM((_GROUPS, _ROWS, 512), f32),
            pltpu.VMEM((2, 2, 256, 512), f32),
            pltpu.VMEM((4, 2, 16, _COMBS * _COMB_ROWS, _LANES), f32),
            pltpu.VMEM((_GROUPS, 4, _ROWS, _LANES), bf16),
            pltpu.VMEM((_GROUPS, 8, _ROWS, _LANES), f32),
            pltpu.VMEM((_GROUPS, 8, _ROWS, _LANES), bf16),
            pltpu.VMEM((tiles, _ROWS, _LANES), f32),
            pltpu.VMEM((tiles, _ROWS, _LANES), bf16),
            pltpu.VMEM((2, tiles, _ROWS, _LANES), bf16),
            pltpu.SemaphoreType.DMA((_GROUPS + 12,)),
            pltpu.SemaphoreType.DMA((sends,)),
            pltpu.SemaphoreType.DMA((receives,)),
        ],
        compiler_params=pltpu.CompilerParams(
            collective_id=0, disable_semaphore_checks=True),
    )(x, W1, W2.reshape(32, _COMBS * _COMB_ROWS, 512))
```
